```python
import numpy as np

kernel_name = "dist_moe_shared_ep_outshard_n256_d128_e2_h256"

def setup_inputs():
    x = np.random.randn(256, 128).astype(np.float32)
    router_W = np.random.randn(128, 8).astype(np.float32) * 0.1
    scores64 = x.astype(np.float64) @ router_W.astype(np.float64)
    route_idx = np.argsort(-scores64, axis=-1)[:, :1].astype(np.int32)
    expert_W = np.random.randn(8, 128, 256).astype(np.float32) * 0.02
    shared_W = np.random.randn(128, 256).astype(np.float32) * 0.02
    return {"x": x, "router_W": router_W, "route_idx": route_idx, "expert_W": expert_W, "shared_W": shared_W}

def reference(x, router_W, route_idx, expert_W, shared_W):
    scores = x @ router_W
    s_max = scores.max(axis=-1, keepdims=True)
    probs = np.exp(scores - s_max)
    probs = probs / probs.sum(axis=-1, keepdims=True)
    shared = x @ shared_W
    out = np.zeros((256, 256), dtype=np.float32)
    for i in range(256):
        e = int(route_idx[i, 0])
        out[i] = shared[i] + probs[i, e] * (x[i] @ expert_W[e])
    return out
```

```python
import jax
import jax.numpy as jnp
from jax import lax
from jax.experimental import pallas as pl
from jax.experimental.pallas import tpu as pltpu

N, D, H, E, NDEV = 256, 128, 256, 8, 4
B = N // NDEV
MESH = pl.DeviceIdType.MESH
f32, bf16, i32 = jnp.float32, jnp.bfloat16, jnp.int32
HI = -65536


def pack(y):
    r = lax.bitcast_convert_type(y.astype(bf16).astype(f32), i32)
    return lax.shift_right_logical(r[:, :128], 16) | (r[:, 128:] & HI)


def body(x, rw, ri, ew, sw, o, xv, rwv, riv, wv, swv, sb, rb, pt, ris, lst, sems):
    me = lax.axis_index("i")
    blk = lambda k: pl.ds(pl.multiple_of(((me + k) % NDEV) * B, B), B)
    c_idx = pltpu.async_copy(ri, ris, sems.at[0])
    c_a = [pltpu.async_copy(x.at[blk(2)], xv.at[pl.ds(0, B)], sems.at[1]),
           pltpu.async_copy(ew.at[0], wv.at[0], sems.at[1])]
    c_b = pltpu.async_copy(ew.at[1], wv.at[1], sems.at[2])
    bar = pltpu.get_barrier_semaphore()
    for k in (2, 1, 3):
        pl.semaphore_signal(bar, inc=1, device_id=((me + k) % NDEV,), device_id_type=MESH)
    c_c = [pltpu.async_copy(x.at[blk(k)], xv.at[pl.ds(j * B, B)], sems.at[3]) for j, k in ((1, 1), (2, 3), (3, 0))]
    c_c += [pltpu.async_copy(sw, swv, sems.at[3]), pltpu.async_copy(rw, rwv, sems.at[3]),
            pltpu.async_copy(ri, riv, sems.at[3])]
    ssem, rsem = sems.at[4], sems.at[5]

    def row_copy(s, d, dev):
        return pltpu.make_async_remote_copy(sb.at[pl.ds(s, 1)], rb.at[pl.ds(d, 1)], ssem, rsem, (dev,), MESH)

    c_idx.wait()
    base = ((me + 2) % NDEV) * B
    n0 = n1 = jnp.int32(0)
    for t in range(B):
        e = ris[0, base + t] & 7
        lst[n0] = t
        lst[B + n1] = t
        n0 = n0 + (e == 2 * me).astype(i32)
        n1 = n1 + (e == 2 * me + 1).astype(i32)

    for c in c_a:
        c.wait()
    xd = xv[pl.ds(0, B), :].astype(bf16)
    w0 = wv[0].astype(bf16)
    sb[pl.ds(0, B), :] = pack(jnp.dot(xd, w0, preferred_element_type=f32))
    pl.semaphore_wait(bar, 3)
    diag = (me + 2) % NDEV

    @pl.loop(0, n0)
    def _(j):
        r = lst[j]
        row_copy(r, r, diag).start()

    c_b.wait()
    w1 = wv[1].astype(bf16)
    sb[pl.ds(N, B), :] = pack(jnp.dot(xd, w1, preferred_element_type=f32))

    @pl.loop(0, n1)
    def _(j):
        r = lst[B + j]
        row_copy(N + r, r, diag).start()

    for c in c_c:
        c.wait()
    xr = xv[pl.ds(B, 3 * B), :].astype(bf16)
    sb[pl.ds(B, 3 * B), :] = pack(jnp.dot(xr, wv[0].astype(bf16), preferred_element_type=f32))
    sb[pl.ds(N + B, 3 * B), :] = pack(jnp.dot(xr, wv[1].astype(bf16), preferred_element_type=f32))
    ns = []
    for j, k in ((1, 1), (2, 3), (3, 0)):
        bs = ((me + k) % NDEV) * B
        n = jnp.int32(0)
        for t in range(B):
            e = ris[0, bs + t] & 7
            lst[(j + 1) * B + n] = t + (e & 1) * N
            n = n + ((e >> 1) == me).astype(i32)
        ns.append(n)
    for (j, k), n in zip(((1, 1), (2, 3), (3, 0)), ns):
        @pl.loop(0, n)
        def _(q):
            r = lst[(j + 1) * B + q]
            row_copy(r + j * B, r & (B - 1), (me + k) % NDEV).start()

    xo = xv[pl.ds(2 * B, 2 * B), :]
    sT = lax.dot_general(rwv[...], xo, (((1,), (1,)), ((), ())), preferred_element_type=f32,
                         precision=lax.Precision.HIGHEST)
    idx = riv[...] & 7
    half = jnp.where(me >= 2, idx[:, 128:], idx[:, :128])
    half = jnp.broadcast_to(half, (E, 128))
    half = jnp.where(me % 2 == 1, half, pltpu.roll(half, 64, 1))
    ex = jnp.exp(sT - jnp.max(sT, axis=0, keepdims=True))
    sel = lax.broadcasted_iota(i32, (E, 128), 0) == half
    p = jnp.sum(jnp.where(sel, ex, 0.0), axis=0, keepdims=True) / jnp.sum(ex, axis=0, keepdims=True)
    pT = jnp.broadcast_to(p, (128, 128)).T[B:, :]
    sh = jnp.dot(xo[B:].astype(bf16), swv[...].astype(bf16), preferred_element_type=f32)

    @pl.loop(0, n0 + n1 + ns[0] + ns[1] + ns[2])
    def _(j):
        row_copy(0, 0, me).wait_send()

    pltpu.make_async_copy(rb, rb, rsem).wait()
    w = rb[...]
    o[:, :128] = sh[:, :128] + pT * lax.bitcast_convert_type(w << 16, f32)
    o[:, 128:] = sh[:, 128:] + pT * lax.bitcast_convert_type(w & HI, f32)


def pallas_dist_moe_shared_ep_outshard_n256_d128_e2_h256_kernel(x, router_W, route_idx, expert_W, shared_W):
    return pl.pallas_call(
        body,
        out_shape=jax.ShapeDtypeStruct((B, H), f32),
        in_specs=[pl.BlockSpec(memory_space=pltpu.HBM)] * 5,
        out_specs=pl.BlockSpec(memory_space=pltpu.VMEM),
        scratch_shapes=[pltpu.VMEM((N, D), f32), pltpu.VMEM((E, D), f32), pltpu.VMEM((1, N), i32),
                        pltpu.VMEM((2, D, H), f32), pltpu.VMEM((D, H), f32),
                        pltpu.VMEM((2 * N, 128), i32), pltpu.VMEM((B, 128), i32), pltpu.VMEM((N, D), f32),
                        pltpu.SMEM((1, N), i32), pltpu.SMEM((5 * B,), i32),
                        pltpu.SemaphoreType.DMA((6,))],
        compiler_params=pltpu.CompilerParams(collective_id=0, disable_bounds_checks=True, disable_semaphore_checks=True),
    )(x, router_W.T, route_idx.reshape(1, N), expert_W, shared_W)
```

```python
import jax
import jax.numpy as jnp
from jax import lax
from jax.experimental import pallas as pl
from jax.experimental.pallas import tpu as pltpu

N_TOK, D_IN, D_OUT, N_EXP, N_DEV = 256, 128, 256, 8, 4
BLK = N_TOK // N_DEV
GRP = 32
N_GRP = N_TOK // GRP
LANES = 128
DIAG, NBR_A, NBR_B, SELF = range(4)
HIGH_HALF = -(1 << 16)

f32, bf16, i32 = jnp.float32, jnp.bfloat16, jnp.int32
MESH = pl.DeviceIdType.MESH


def _pack(y):
    r = lax.bitcast_convert_type(y.astype(bf16).astype(f32), i32)
    return lax.shift_right_logical(r[:, :LANES], 16) | (r[:, LANES:] & HIGH_HALF)


def _unpack(w):
    return (
        lax.bitcast_convert_type(w << 16, f32),
        lax.bitcast_convert_type(w & HIGH_HALF, f32),
    )


def _split(v):
    hi = v.astype(bf16).astype(f32)
    return jnp.concatenate([hi, v - hi], axis=0).astype(bf16)


class _RowQueue:
    def __init__(self, mask, count, row_copy):
        self.mask, self.count, self.row_copy = mask, count, row_copy
        self.started = 0

    def start_next(self):
        rest = self.mask & (self.mask - 1)
        row = lax.clz(self.mask ^ rest)
        pl.when(self.count > self.started)(lambda: self.row_copy(row).start())
        self.mask, self.started = rest, self.started + 1

    def start_remaining(self):
        def step(_, mask):
            rest = mask & (mask - 1)
            self.row_copy(lax.clz(mask ^ rest)).start()
            return rest

        lax.fori_loop(self.started, self.count, step, self.mask)


def _start_some(queues, rounds):
    for _ in range(rounds):
        for q in queues:
            q.start_next()


def _start_remaining(queues):
    for q in queues:
        q.start_remaining()


def _body(
    x_hbm, rw_hbm, idx_hbm, ew_hbm, sw_hbm, out_ref,
    x_v, rw_v, idx_v, ew_v, sw_v, send_bufs, recv_bufs, masks, counts,
    load_sems, send_sem, recv_sems,
):
    load_idx = pltpu.async_copy(idx_hbm, idx_v, load_sems.at[0])
    load_w0 = pltpu.async_copy(ew_hbm.at[0], ew_v.at[0], load_sems.at[1])
    me = lax.axis_index("i")
    peers = [me ^ 2, 1 - (me & 1), 3 - (me & 1), me]

    def load_x(j, sem, priority):
        rows = pl.ds(pl.multiple_of(peers[j] * BLK, BLK), BLK)
        return pltpu.async_copy(
            x_hbm.at[rows], x_v.at[pl.ds(j * BLK, BLK)], sem, priority=priority
        )

    load_xd = load_x(DIAG, load_sems.at[1], 0)
    load_w1 = pltpu.async_copy(ew_hbm.at[1], ew_v.at[1], load_sems.at[2], priority=1)
    barrier = pltpu.get_barrier_semaphore()
    for j in (DIAG, NBR_A, NBR_B):
        pl.semaphore_signal(barrier, inc=1, device_id=(peers[j],), device_id_type=MESH)

    sub = lax.broadcasted_iota(i32, (8, LANES), 0)
    lane = lax.broadcasted_iota(i32, (8, LANES), 1)
    bit = jnp.where(
        (lane >> 5) == (sub & 3), (1 << (15 - (lane & 15))).astype(f32), 0.0
    )
    bit_hi = jnp.where((lane & 16) == 0, bit, 0.0)
    bit_lo = jnp.where((lane & 16) == 0, 0.0, bit)
    wanted = 2 * me + (sub >> 2)
    load_idx.wait()
    idx = idx_v[...] & (N_EXP - 1)
    for h in range(N_TOK // LANES):
        hit = jnp.broadcast_to(idx[:, h * LANES:(h + 1) * LANES], (8, LANES)) == wanted
        hi = jnp.sum(jnp.where(hit, bit_hi, 0.0), axis=1, keepdims=True).astype(i32)
        lo = jnp.sum(jnp.where(hit, bit_lo, 0.0), axis=1, keepdims=True).astype(i32)
        word = (hi << 16) | lo
        count = lax.population_count(word)
        for s in range(8):
            slot = (s // 4) * N_GRP + 4 * h + s % 4
            masks[slot] = word[s, 0]
            counts[slot] = count[s, 0]

    def row_copy(j, e, g, row):
        src = send_bufs[j][e].at[pl.ds(g * GRP + row, 1)]
        dst = recv_bufs[g].at[pl.ds(row, 1)]
        if j == SELF:
            return pltpu.make_async_copy(src, dst, recv_sems.at[g])
        return pltpu.make_async_remote_copy(
            src, dst, send_sem, recv_sems.at[g], (peers[j],), MESH
        )

    def queue(j, e, g):
        slot = e * N_GRP + 2 * peers[j] + g
        return _RowQueue(masks[slot], counts[slot], lambda row: row_copy(j, e, g, row))

    def queues(j):
        return [queue(j, e, g) for g in range(2) for e in range(2)]

    q_e0 = [queue(DIAG, 0, g) for g in range(2)]
    q_e1 = [queue(DIAG, 1, g) for g in range(2)]

    load_w0.wait()
    load_xd.wait()
    load_rest = [load_x(j, load_sems.at[3], 1) for j in (NBR_A, NBR_B, SELF)] + [
        pltpu.async_copy(sw_hbm, sw_v, load_sems.at[3], priority=1),
        pltpu.async_copy(rw_hbm, rw_v, load_sems.at[3], priority=1),
    ]
    xd = x_v[pl.ds(DIAG * BLK, BLK), :].astype(bf16)

    def diag_rows(e):
        w = ew_v[e].astype(bf16)
        ys = [
            _pack(jnp.dot(
                jnp.concatenate([xd[r:r + 16], xd[GRP + r:GRP + r + 16]], axis=0),
                w, preferred_element_type=f32,
            ))
            for r in (0, 16)
        ]
        return [jnp.concatenate([y[r:r + 16] for y in ys], axis=0) for r in (0, 16)]

    send_bufs[DIAG][0][...] = jnp.concatenate(diag_rows(0), axis=0)
    pl.semaphore_wait(barrier, N_DEV - 1)
    load_w1.wait()
    y = diag_rows(1)
    _start_some(q_e0, 6)
    send_bufs[DIAG][1][:GRP] = y[0]
    _start_some(q_e1[:1], 2)
    send_bufs[DIAG][1][GRP:] = y[1]
    _start_some(q_e1[:1], 1)
    _start_remaining(q_e1 + q_e0)

    for load in load_rest:
        load.wait()
    q_a = queues(NBR_A)
    xr = x_v[pl.ds(NBR_A * BLK, 3 * BLK), :].astype(bf16)
    ys = [
        _pack(jnp.dot(xr, ew_v[e].astype(bf16), preferred_element_type=f32))
        for e in range(2)
    ]
    for e in range(2):
        send_bufs[NBR_A][e][...] = ys[e][:BLK]
    _start_some(q_a, 5)
    for e in range(2):
        send_bufs[NBR_B][e][...] = ys[e][BLK:2 * BLK]
        send_bufs[SELF][e][...] = ys[e][2 * BLK:]
    _start_remaining(q_a)

    xo = x_v[pl.ds(SELF * BLK, BLK), :]
    scores = lax.dot_general(
        _split(rw_v[...]), _split(xo), (((1,), (1,)), ((), ())),
        preferred_element_type=f32,
    )
    scores = scores[:N_EXP] + scores[N_EXP:]
    scores = scores + pltpu.roll(scores, BLK, 1)
    ex = jnp.exp(scores - jnp.max(scores, axis=0, keepdims=True))
    routed = jnp.broadcast_to(
        jnp.where(me >= 2, idx[:, LANES:], idx[:, :LANES]), (N_EXP, LANES)
    )
    gate = jnp.sum(jnp.where(sub == routed, ex, 0.0), axis=0, keepdims=True) / jnp.sum(
        ex, axis=0, keepdims=True
    )
    own_lane = lax.broadcasted_iota(i32, (BLK, LANES), 1) == (
        lax.broadcasted_iota(i32, (BLK, LANES), 0) + (me & 1) * BLK
    )
    gate = jnp.broadcast_to(
        jnp.sum(jnp.where(own_lane, gate, 0.0), axis=1, keepdims=True), (BLK, LANES)
    )
    shared = jnp.dot(
        xo.astype(bf16), sw_v[...].astype(bf16), preferred_element_type=f32
    )
    q_b = queues(NBR_B)
    _start_some(q_b, 5)
    q_self = queues(SELF)
    _start_some(q_self, 5)
    _start_remaining(q_b + q_self)

    n_sent = sum(q.count for q in q_e0 + q_e1 + q_a + q_b)

    @pl.loop(0, n_sent >> 3)
    def _(_):
        for _ in range(8):
            row_copy(DIAG, 0, 0, 0).wait_send()

    @pl.loop(0, n_sent & 7)
    def _(_):
        row_copy(DIAG, 0, 0, 0).wait_send()

    for g in range(2):
        pltpu.make_async_copy(recv_bufs[g], recv_bufs[g], recv_sems.at[g]).wait()
        rows = slice(g * GRP, (g + 1) * GRP)
        y_lo, y_hi = _unpack(recv_bufs[g][...])
        out_ref[rows, :LANES] = shared[rows, :LANES] + gate[rows] * y_lo
        out_ref[rows, LANES:] = shared[rows, LANES:] + gate[rows] * y_hi


def pallas_dist_moe_shared_ep_outshard_n256_d128_e2_h256_kernel(
    x: jax.Array,
    router_W: jax.Array,
    route_idx: jax.Array,
    expert_W: jax.Array,
    shared_W: jax.Array,
):
    return pl.pallas_call(
        _body,
        out_shape=jax.ShapeDtypeStruct((BLK, D_OUT), f32),
        in_specs=[pl.BlockSpec(memory_space=pltpu.HBM)] * 5,
        out_specs=pl.BlockSpec(memory_space=pltpu.VMEM),
        scratch_shapes=[
            pltpu.VMEM((N_TOK, D_IN), f32),
            pltpu.VMEM((N_EXP, D_IN), f32),
            pltpu.VMEM((1, N_TOK), i32),
            pltpu.VMEM((2, D_IN, D_OUT), f32),
            pltpu.VMEM((D_IN, D_OUT), f32),
            [[pltpu.VMEM((BLK, LANES), i32)] * 2] * N_DEV,
            [pltpu.VMEM((GRP, LANES), i32)] * 2,
            pltpu.SMEM((2 * N_GRP,), i32),
            pltpu.SMEM((2 * N_GRP,), i32),
            pltpu.SemaphoreType.DMA((4,)),
            pltpu.SemaphoreType.DMA,
            pltpu.SemaphoreType.DMA((2,)),
        ],
        compiler_params=pltpu.CompilerParams(
            collective_id=0,
            disable_bounds_checks=True,
            disable_semaphore_checks=True,
        ),
    )(x, router_W.T, route_idx.reshape(1, N_TOK), expert_W, shared_W)
```
